```python
import numpy as np

kernel_name = "dist_rope_attn_qseq_b2_sq128_d512_hq4_dh64"

def setup_inputs():
    x = np.random.randn(2, 512, 512).astype(np.float32)
    Wq = np.random.randn(512, 256).astype(np.float32) * 0.02
    Wk = np.random.randn(512, 256).astype(np.float32) * 0.02
    Wv = np.random.randn(512, 256).astype(np.float32) * 0.02
    Wo = np.random.randn(256, 512).astype(np.float32) * 0.02
    return {"x": x, "Wq": Wq, "Wk": Wk, "Wv": Wv, "Wo": Wo}

def reference(x, Wq, Wk, Wv, Wo):
    B, Sq, Hq, Dh = 2, 512, 4, 64
    inv = 1.0 / (10000.0 ** (np.arange(0, Dh, 2) / Dh))
    pos = np.arange(Sq)[:, None] * inv[None, :]
    cos = np.repeat(np.cos(pos), 2, axis=-1).astype(np.float32)
    sin = np.repeat(np.sin(pos), 2, axis=-1).astype(np.float32)
    def rot(t):
        t2 = t.reshape(B, Sq, Hq, Dh // 2, 2)
        t_r = np.stack([-t2[..., 1], t2[..., 0]], axis=-1).reshape(B, Sq, Hq, Dh)
        return t * cos[None, :, None, :] + t_r * sin[None, :, None, :]
    Q = rot((x @ Wq).reshape(B, Sq, Hq, Dh))
    K = rot((x @ Wk).reshape(B, Sq, Hq, Dh))
    V = (x @ Wv).reshape(B, Sq, Hq, Dh)
    s = np.einsum('bihd,bjhd->bhij', Q, K).astype(np.float32) * 0.125
    s_max = s.max(axis=-1, keepdims=True)
    w = np.exp(s - s_max)
    w = w / w.sum(axis=-1, keepdims=True)
    ctx = np.einsum('bhij,bjhd->bihd', w, V).reshape(B, Sq, Hq * Dh)
    return ctx @ Wo
```

```python
import functools
import math
import jax
import jax.numpy as jnp
from jax import lax
from jax.experimental import pallas as pl
from jax.experimental.pallas import tpu as pltpu

F32 = jnp.float32
BF16 = jnp.bfloat16
MESH = pl.DeviceIdType.MESH
ROWS = 128
DH = 64
LOG2E = 1.4426950408889634
QSCALE = 0.125 * LOG2E


def _body(x_hbm, wq_hbm, wk_hbm, wv_hbm, wo_hbm, out_hbm,
          x_v, w_v, wo_v, snd, rcv, csnd, crcv,
          in_sems, s_sems, r_sems, sc_sems, rc_sems):
    me = lax.axis_index("i")
    b0 = me // 2
    p0 = me % 2

    def wcopy(w_hbm, p, slot):
        return pltpu.make_async_copy(
            w_hbm.at[:, pl.ds(pl.multiple_of(p * 128, 128), 128)], w_v.at[slot], in_sems.at[1 + slot])
    x_cp = pltpu.make_async_copy(x_hbm, x_v, in_sems.at[0])
    x_cp.start()
    w_cps = [wcopy(wk_hbm, 1 - p0, 0), wcopy(wk_hbm, p0, 1),
             wcopy(wv_hbm, 1 - p0, 2), wcopy(wv_hbm, p0, 3),
             wcopy(wq_hbm, 1 - p0, 4), wcopy(wq_hbm, p0, 5)]
    for c in w_cps:
        c.start()
    wo_cp = pltpu.make_async_copy(wo_hbm, wo_v, in_sems.at[7])
    wo_cp.start()

    bar = pltpu.get_barrier_semaphore()
    for k in (1, 2, 3):
        pl.semaphore_signal(bar, inc=1, device_id=(me ^ k,), device_id_type=MESH)

    lane = lax.broadcasted_iota(jnp.int32, (ROWS, 128), 1)
    row = lax.broadcasted_iota(jnp.int32, (ROWS, 128), 0)
    fidx = ((lane % DH) // 2).astype(F32)
    inv = jnp.exp(fidx * (-math.log(10000.0) / (DH // 2)))
    ang = (row + me * ROWS).astype(F32) * inv
    cos_t = jnp.cos(ang)
    sin_t = jnp.sin(ang)
    even = (lane % 2) == 0
    sin_s = jnp.where(even, -sin_t, sin_t)
    lo = lane < DH

    def rope(t):
        sw = jnp.where(even, pltpu.roll(t, 127, 1), pltpu.roll(t, 1, 1))
        return t * cos_t + sw * sin_s

    x_cp.wait()
    xb = x_v[...].reshape(2 * ROWS, 512).astype(BF16)

    def proj(slot):
        w_cps[slot].wait()
        return jnp.dot(xb, w_v[slot].astype(BF16), preferred_element_type=F32)

    rdmas = []

    def send(kind, blk, k):
        cp = pltpu.make_async_remote_copy(
            snd.at[kind, blk], rcv.at[kind, k], s_sems.at[kind, k - 1], r_sems.at[kind, k - 1],
            device_id=(me ^ k,), device_id_type=MESH)
        cp.start()
        rdmas.append(cp)

    def emit(kind, half, y, fn):
        for b in range(2):
            snd[kind, 2 * half + b] = fn(y[b * ROWS:(b + 1) * ROWS]).astype(BF16)

    ident = lambda t: t
    ropeq = lambda t: rope(t) * QSCALE
    first = True
    for kind, fn in ((0, rope), (1, ident), (2, ropeq)):
        y = proj(2 * kind)
        emit(kind, 0, y, fn)
        if first:
            pl.semaphore_wait(bar, 3)
            first = False
        send(kind, b0, 1)
        send(kind, 1 - b0, 3)
        y = proj(2 * kind + 1)
        emit(kind, 1, y, fn)
        send(kind, 2 + 1 - b0, 2)
        rcv[kind, 0] = snd[kind, 2 + b0]

    def recv_wait(kind, k):
        pltpu.make_async_remote_copy(
            snd.at[kind, 0], rcv.at[kind, k], s_sems.at[kind, k - 1], r_sems.at[kind, k - 1],
            device_id=(me,), device_id_type=MESH).wait_recv()

    for kind in (0, 1):
        for k in (1, 2, 3):
            recv_wait(kind, k)
    kk = rcv[0].reshape(4 * ROWS, 128)
    vv = rcv[1].reshape(4 * ROWS, 128)

    csends = []
    for k in (0, 2, 1, 3):
        if k:
            recv_wait(2, k)
        q = rcv[2, k]
        zero = jnp.zeros_like(q)
        qs = jnp.concatenate([jnp.where(lo, q, zero), jnp.where(lo, zero, q)], axis=0)
        s = lax.dot_general(qs, kk, (((1,), (1,)), ((), ())), preferred_element_type=F32)
        m = jnp.max(s, axis=1, keepdims=True)
        p = jnp.exp2(s - m)
        l = jnp.sum(p, axis=1, keepdims=True)
        o = jnp.dot(p.astype(BF16), vv, preferred_element_type=F32)
        o = o * (1.0 / l)
        ctx = jnp.where(lo, o[:ROWS], o[ROWS:]).astype(BF16)
        if k == 0:
            crcv[b0, :, pl.ds(pl.multiple_of(p0 * 128, 128), 128)] = ctx
        else:
            csnd[k - 1] = ctx
            cp = pltpu.make_async_remote_copy(
                csnd.at[k - 1], crcv.at[b0, :, pl.ds(pl.multiple_of(p0 * 128, 128), 128)],
                sc_sems.at[k - 1], rc_sems.at[k - 1], device_id=(me ^ k,), device_id_type=MESH)
            cp.start()
            csends.append(cp)

    wo_cp.wait()
    wo = wo_v[...].astype(BF16)

    def cwait(k):
        pltpu.make_async_remote_copy(
            csnd.at[0], crcv.at[0, :, pl.ds(0, 128)], sc_sems.at[k - 1], rc_sems.at[k - 1],
            device_id=(me,), device_id_type=MESH).wait_recv()

    cwait(1)
    out_hbm[b0] = jnp.dot(crcv[b0], wo, preferred_element_type=F32)
    cwait(2)
    cwait(3)
    out_hbm[1 - b0] = jnp.dot(crcv[1 - b0], wo, preferred_element_type=F32)
    for cp in rdmas + csends:
        cp.wait_send()


def pallas_dist_rope_attn_qseq_b2_sq128_d512_hq4_dh64_kernel(x, Wq, Wk, Wv, Wo):
    any_spec = pl.BlockSpec(memory_space=pltpu.HBM)
    return pl.pallas_call(
        _body,
        out_shape=pltpu.VMEM(x.shape, F32),
        in_specs=[any_spec] * 5,
        out_specs=pl.BlockSpec(memory_space=pltpu.VMEM),
        scratch_shapes=[
            pltpu.VMEM((2, ROWS, 512), F32),
            pltpu.VMEM((6, 512, 128), F32),
            pltpu.VMEM((256, 512), F32),
            pltpu.VMEM((3, 4, ROWS, 128), BF16),
            pltpu.VMEM((3, 4, ROWS, 128), BF16),
            pltpu.VMEM((3, ROWS, 128), BF16),
            pltpu.VMEM((2, ROWS, 256), BF16),
            pltpu.SemaphoreType.DMA((8,)),
            pltpu.SemaphoreType.DMA((3, 3)),
            pltpu.SemaphoreType.DMA((3, 3)),
            pltpu.SemaphoreType.DMA((3,)),
            pltpu.SemaphoreType.DMA((3,)),
        ],
        compiler_params=pltpu.CompilerParams(collective_id=0),
    )(x, Wq, Wk, Wv, Wo)
```

```python
import math

import jax
import jax.numpy as jnp
from jax import lax
from jax.experimental import pallas as pl
from jax.experimental.pallas import tpu as pltpu

F32 = jnp.float32
BF16 = jnp.bfloat16
MESH = pl.DeviceIdType.MESH

ROWS = 128
DM = 512
DH = 64
NT = (((1,), (1,)), ((), ()))
QSCALE = 0.125 * math.log2(math.e)

TK, TV, TQ = 0, 1, 2
OWN, Y, D, X = 0, 1, 2, 3
REL = {OWN: (0, 0), Y: (1, 0), D: (1, 1), X: (0, 1)}
SLOT = {rel: k for k, rel in REL.items()}

LOADS = (
    (TK, 1), ("x", 1), (TK, 0), ("x", 0), (TQ, 1), (TV, 0), (TV, 1), (TQ, 0), ("wo",),
)
N_LOADS = len(LOADS)
SEM_K, SEM_V, SEM_Q, SEM_SEND, SEM_GATE = (N_LOADS + i for i in (0, 1, 2, 5, 6))
N_SCOPED_SEMS = N_LOADS + 7


def _lo_lanes(rows):
    return lax.broadcasted_iota(jnp.int32, (rows, 128), 1) < DH


def _wait_bytes_of(ref, sem):
    pltpu.make_async_copy(ref, ref, sem).wait()


def _reciprocal(v):
    r = pl.reciprocal(v, approx=True)
    return r * (2.0 - v * r)


def _ctx_copy(csnd, crcv, send_sem, c_sems, me, k):
    return pltpu.make_async_remote_copy(
        csnd.at[k - 1], crcv.at[k], send_sem, c_sems.at[k - 1],
        device_id=(me ^ k,), device_id_type=MESH)


def _exchange_and_attend(x_hbm, wq_hbm, wk_hbm, wv_hbm, wo_hbm,
                         x_v, xb_v, w_v, wo_v, wob, snd, rcv, csnd, crcv, acc, pst, lst,
                         c_send_sem, c_sems, sems):
    me = lax.axis_index("i")
    b0 = (me ^ (me >> 1)) & 1
    p0 = me >> 1
    w_hbm = {TK: wk_hbm, TV: wv_hbm, TQ: wq_hbm}

    loads = {}
    for n, ld in enumerate(LOADS):
        if ld[0] == "x":
            flip = ld[1]
            cp = pltpu.make_async_copy(
                x_hbm.at[(1 - b0) if flip else b0], x_v.at[flip], sems.at[n])
        elif ld[0] == "wo":
            cp = pltpu.make_async_copy(wo_hbm, wo_v, sems.at[n])
        else:
            kind, flip = ld
            pair = (1 - p0) if flip else p0
            cp = pltpu.make_async_copy(
                w_hbm[kind].at[:, pl.ds(pl.multiple_of(pair * 128, 128), 128)],
                w_v.at[kind, flip], sems.at[n])
        cp.start()
        loads[ld] = cp

    barrier = pltpu.get_barrier_semaphore()
    for k in (1, 2, 3):
        pl.semaphore_signal(barrier, inc=1, device_id=(me ^ k,), device_id_type=MESH)

    lane = lax.broadcasted_iota(jnp.int32, (ROWS, 128), 1)
    row = lax.broadcasted_iota(jnp.int32, (ROWS, 128), 0)
    freq_idx = ((lane % DH) // 2).astype(F32)
    inv_freq = jnp.exp(freq_idx * (-math.log(10000.0) / (DH // 2)))
    angle = (row + me * ROWS).astype(F32) * inv_freq
    cos_t = jnp.cos(angle)
    sin_t = jnp.sin(angle)
    even = (lane % 2) == 0
    sin_signed = jnp.where(even, -sin_t, sin_t)

    def rope(t):
        swapped = jnp.where(even, pltpu.roll(t, 127, 1), pltpu.roll(t, 1, 1))
        return t * cos_t + swapped * sin_signed

    post = {TK: rope, TV: lambda t: t, TQ: lambda t: rope(t) * QSCALE}

    ready = set()
    sends = []
    gate = []

    def send(kind, k, gated=False):
        if "barrier" not in ready:
            pl.semaphore_wait(barrier, 3)
            ready.add("barrier")
        recv_sem = sems.at[{TK: SEM_K, TV: SEM_V, TQ: SEM_Q + k - 1}[kind]]
        cp = pltpu.make_async_remote_copy(
            snd.at[kind, k - 1], rcv.at[kind, k],
            sems.at[SEM_GATE if gated else SEM_SEND], recv_sem,
            device_id=(me ^ k,), device_id_type=MESH)
        cp.start()
        (gate if gated else sends).append(cp)

    def project(kind, batch_flips, pair_flip, send_to=(), gated_slot=None):
        if (kind, pair_flip) not in ready:
            loads[(kind, pair_flip)].wait()
            ready.add((kind, pair_flip))
        for flip in batch_flips:
            if ("x", flip) not in ready:
                loads[("x", flip)].wait()
                xb_v[flip] = x_v[flip].astype(BF16)
                ready.add(("x", flip))
        order = sorted(batch_flips)
        xin = xb_v[...].reshape(2 * ROWS, DM) if len(order) == 2 else xb_v[order[0]]
        y = jnp.dot(xin, w_v[kind, pair_flip].astype(BF16), preferred_element_type=F32)
        for flip in batch_flips:
            i = order.index(flip)
            k = SLOT[(flip, pair_flip)]
            blk = post[kind](y[i * ROWS:(i + 1) * ROWS]).astype(BF16)
            if k == OWN:
                rcv[kind, OWN] = blk
            else:
                snd[kind, k - 1] = blk
                if k in send_to:
                    send(kind, k, gated=(k == gated_slot))

    project(TK, (1,), 1, (D,))
    project(TK, (1,), 0, (Y,))
    project(TK, (0,), 1, (X,))
    project(TQ, (1,), 1, (D,))
    project(TV, (1,), 0, (Y,))
    project(TV, (1, 0), 1, (D, X), gated_slot=X)
    project(TQ, (0,), 1, (X,))
    project(TV, (0,), 0)
    project(TK, (0,), 0)
    project(TQ, (1, 0), 0)

    def stacked_q(k):
        q = rcv[TQ, k]
        lo = _lo_lanes(ROWS)
        zero = jnp.zeros_like(q)
        return jnp.concatenate([jnp.where(lo, q, zero), jnp.where(lo, zero, q)], axis=0)

    def scores(k):
        keys = rcv[TK].reshape(4 * ROWS, 128)
        return lax.dot_general(stacked_q(k), keys, NT, preferred_element_type=F32)

    def softmax_parts(s):
        m = jnp.max(s, axis=1, keepdims=True)
        p = jnp.exp2(s - m)
        return p.astype(BF16), _reciprocal(jnp.sum(p, axis=1, keepdims=True))

    def values():
        return rcv[TV].reshape(4 * ROWS, 128)

    def finish(k, o, inv_l):
        o = o * inv_l
        ctx = jnp.where(_lo_lanes(ROWS), o[:ROWS], o[ROWS:]).astype(BF16)
        if k == OWN:
            crcv[OWN] = ctx
        else:
            csnd[k - 1] = ctx
            _ctx_copy(csnd, crcv, c_send_sem, c_sems, me, k).start()

    def softmax_stage(k, slot):
        p, inv_l = softmax_parts(scores(k))
        pst[slot] = p
        lst[slot] = jnp.broadcast_to(inv_l, (2 * ROWS, 128))

    def value_stage(k, slot):
        o = jnp.dot(pst[slot], values(), preferred_element_type=F32)
        finish(k, o, lst[slot])

    _wait_bytes_of(rcv.at[TK, pl.ds(1, 3)], sems.at[SEM_K])
    softmax_stage(OWN, 0)

    gate[0].wait_send()
    send(TQ, Y)

    loads[("wo",)].wait()
    wob[0] = wo_v[pl.ds(pl.multiple_of(p0 * 128, 128), 128), :].astype(BF16)
    wob[1] = wo_v[pl.ds(pl.multiple_of((1 - p0) * 128, 128), 128), :].astype(BF16)

    _wait_bytes_of(rcv.at[TQ, D], sems.at[SEM_Q + D - 1])
    softmax_stage(D, 1)
    _wait_bytes_of(rcv.at[TV, pl.ds(1, 3)], sems.at[SEM_V])
    value_stage(D, 1)

    _wait_bytes_of(rcv.at[TQ, X], sems.at[SEM_Q + X - 1])
    _wait_bytes_of(rcv.at[TQ, Y], sems.at[SEM_Q + Y - 1])
    p, inv_l = softmax_parts(scores(X))
    o = jnp.dot(p, values(), preferred_element_type=F32)
    s_next = scores(Y)
    finish(X, o, inv_l)
    p, inv_l = softmax_parts(s_next)
    o = jnp.dot(p, values(), preferred_element_type=F32)
    finish(Y, o, inv_l)

    value_stage(OWN, 0)

    for cp in sends:
        cp.wait_send()


def _kernel_body(x_hbm, wq_hbm, wk_hbm, wv_hbm, wo_hbm, out_ref,
                 x_v, xb_v, w_v, wo_v, wob, snd, rcv, csnd, crcv, acc, pst, lst,
                 c_send_sem, c_sems):
    pl.run_scoped(
        lambda sems: _exchange_and_attend(
            x_hbm, wq_hbm, wk_hbm, wv_hbm, wo_hbm,
            x_v, xb_v, w_v, wo_v, wob, snd, rcv, csnd, crcv, acc, pst, lst,
            c_send_sem, c_sems, sems),
        pltpu.SemaphoreType.DMA((N_SCOPED_SEMS,)))

    me = lax.axis_index("i")
    b0 = (me ^ (me >> 1)) & 1

    def out_part(k):
        return jnp.dot(crcv[k], wob[REL[k][1]], preferred_element_type=F32)

    acc[0] = out_part(OWN)
    _wait_bytes_of(crcv.at[D], c_sems.at[D - 1])
    acc[1] = out_part(D)
    _wait_bytes_of(crcv.at[X], c_sems.at[X - 1])
    out_ref[b0] = acc[0] + out_part(X)
    _wait_bytes_of(crcv.at[Y], c_sems.at[Y - 1])
    out_ref[1 - b0] = acc[1] + out_part(Y)

    for k in (D, X, Y):
        _ctx_copy(csnd, crcv, c_send_sem, c_sems, me, k).wait_send()


def pallas_dist_rope_attn_qseq_b2_sq128_d512_hq4_dh64_kernel(x, Wq, Wk, Wv, Wo):
    hbm = pl.BlockSpec(memory_space=pltpu.HBM)
    return pl.pallas_call(
        _kernel_body,
        out_shape=pltpu.VMEM(x.shape, F32),
        in_specs=[hbm] * 5,
        out_specs=pl.BlockSpec(memory_space=pltpu.VMEM),
        scratch_shapes=[
            pltpu.VMEM((2, ROWS, DM), F32),
            pltpu.VMEM((2, ROWS, DM), BF16),
            pltpu.VMEM((3, 2, DM, 128), F32),
            pltpu.VMEM((256, DM), F32),
            pltpu.VMEM((2, 128, DM), BF16),
            pltpu.VMEM((3, 3, ROWS, 128), BF16),
            pltpu.VMEM((3, 4, ROWS, 128), BF16),
            pltpu.VMEM((3, ROWS, 128), BF16),
            pltpu.VMEM((4, ROWS, 128), BF16),
            pltpu.VMEM((2, ROWS, DM), F32),
            pltpu.VMEM((2, 2 * ROWS, 512), BF16),
            pltpu.VMEM((2, 2 * ROWS, 128), F32),
            pltpu.SemaphoreType.DMA,
            pltpu.SemaphoreType.DMA((3,)),
        ],
        compiler_params=pltpu.CompilerParams(collective_id=0),
    )(x, Wq, Wk, Wv, Wo)
```

```python
import math

import jax
import jax.numpy as jnp
from jax import lax
from jax.experimental import pallas as pl
from jax.experimental.pallas import tpu as pltpu

F32 = jnp.float32
BF16 = jnp.bfloat16
MESH = pl.DeviceIdType.MESH

ROWS = 128
DM = 512
DH = 64
NT = (((1,), (1,)), ((), ()))
QSCALE = 0.125 * math.log2(math.e)

TK, TV, TQ = 0, 1, 2
OWN, Y, D, X = 0, 1, 2, 3
REL = {OWN: (0, 0), Y: (1, 0), D: (1, 1), X: (0, 1)}
SLOT = {rel: k for k, rel in REL.items()}

LOADS = (
    (TK, 1), ("x", 1), (TK, 0), ("x", 0), (TQ, 1), (TV, 0), (TV, 1), (TQ, 0), ("wo",),
)
N_LOADS = len(LOADS)
SEM_K, SEM_V, SEM_Q, SEM_SEND, SEM_GATE = (N_LOADS + i for i in (0, 1, 2, 5, 6))
N_SCOPED_SEMS = N_LOADS + 7

_approx_reciprocal = getattr(pltpu, "reciprocal", None) or pl.reciprocal


def _lo_lanes(rows):
    return lax.broadcasted_iota(jnp.int32, (rows, 128), 1) < DH


def _wait_bytes_of(ref, sem):
    pltpu.make_async_copy(ref, ref, sem).wait()


def _reciprocal(v):
    r = _approx_reciprocal(v, approx=True)
    return r * (2.0 - v * r)


def _ctx_copy(csnd, crcv, send_sem, c_sems, me, k):
    return pltpu.make_async_remote_copy(
        csnd.at[k - 1], crcv.at[k], send_sem, c_sems.at[k - 1],
        device_id=(me ^ k,), device_id_type=MESH)


def _exchange_and_attend(x_hbm, wq_hbm, wk_hbm, wv_hbm, wo_hbm,
                         x_v, xb_v, w_v, wo_v, wob, snd, rcv, csnd, crcv, pst, lst,
                         c_send_sem, c_sems, sems):
    me = lax.axis_index("i")
    b0 = (me ^ (me >> 1)) & 1
    p0 = me >> 1
    w_hbm = {TK: wk_hbm, TV: wv_hbm, TQ: wq_hbm}

    loads = {}
    for n, ld in enumerate(LOADS):
        if ld[0] == "x":
            flip = ld[1]
            cp = pltpu.make_async_copy(
                x_hbm.at[(1 - b0) if flip else b0], x_v.at[flip], sems.at[n])
        elif ld[0] == "wo":
            cp = pltpu.make_async_copy(wo_hbm, wo_v, sems.at[n])
        else:
            kind, flip = ld
            pair = (1 - p0) if flip else p0
            cp = pltpu.make_async_copy(
                w_hbm[kind].at[:, pl.ds(pl.multiple_of(pair * 128, 128), 128)],
                w_v.at[kind, flip], sems.at[n])
        cp.start()
        loads[ld] = cp

    barrier = pltpu.get_barrier_semaphore()
    for k in (1, 2, 3):
        pl.semaphore_signal(barrier, inc=1, device_id=(me ^ k,), device_id_type=MESH)

    lane = lax.broadcasted_iota(jnp.int32, (ROWS, 128), 1)
    row = lax.broadcasted_iota(jnp.int32, (ROWS, 128), 0)
    freq_idx = ((lane % DH) // 2).astype(F32)
    inv_freq = jnp.exp(freq_idx * (-math.log(10000.0) / (DH // 2)))
    angle = (row + me * ROWS).astype(F32) * inv_freq
    cos_t = jnp.cos(angle)
    sin_t = jnp.sin(angle)
    even = (lane % 2) == 0
    sin_signed = jnp.where(even, -sin_t, sin_t)

    def rope(t):
        swapped = jnp.where(even, pltpu.roll(t, 127, 1), pltpu.roll(t, 1, 1))
        return t * cos_t + swapped * sin_signed

    post = {TK: rope, TV: lambda t: t, TQ: lambda t: rope(t) * QSCALE}

    ready = set()
    sends = []
    gate = []

    def send(kind, k, gated=False):
        if "barrier" not in ready:
            pl.semaphore_wait(barrier, 3)
            ready.add("barrier")
        recv_sem = sems.at[{TK: SEM_K, TV: SEM_V, TQ: SEM_Q + k - 1}[kind]]
        cp = pltpu.make_async_remote_copy(
            snd.at[kind, k - 1], rcv.at[kind, k],
            sems.at[SEM_GATE if gated else SEM_SEND], recv_sem,
            device_id=(me ^ k,), device_id_type=MESH)
        cp.start()
        (gate if gated else sends).append(cp)

    def project(kind, batch_flips, pair_flip, send_to=(), gated_slot=None):
        if (kind, pair_flip) not in ready:
            loads[(kind, pair_flip)].wait()
            ready.add((kind, pair_flip))
        for flip in batch_flips:
            if ("x", flip) not in ready:
                loads[("x", flip)].wait()
                xb_v[flip] = x_v[flip].astype(BF16)
                ready.add(("x", flip))
        order = sorted(batch_flips)
        xin = xb_v[...].reshape(2 * ROWS, DM) if len(order) == 2 else xb_v[order[0]]
        y = jnp.dot(xin, w_v[kind, pair_flip].astype(BF16), preferred_element_type=F32)
        for flip in batch_flips:
            i = order.index(flip)
            k = SLOT[(flip, pair_flip)]
            blk = post[kind](y[i * ROWS:(i + 1) * ROWS]).astype(BF16)
            if k == OWN:
                rcv[kind, OWN] = blk
            else:
                snd[kind, k - 1] = blk
                if k in send_to:
                    send(kind, k, gated=(k == gated_slot))

    project(TK, (1,), 1, (D,))
    project(TK, (1,), 0, (Y,))
    project(TK, (0,), 1, (X,))
    project(TQ, (1,), 1, (D,))
    project(TV, (1,), 0, (Y,))
    project(TV, (1, 0), 1, (D, X), gated_slot=X)
    project(TQ, (0,), 1, (X,))
    project(TV, (0,), 0)
    project(TK, (0,), 0)
    project(TQ, (1, 0), 0)

    def stacked_q(k):
        q = rcv[TQ, k]
        lo = _lo_lanes(ROWS)
        zero = jnp.zeros_like(q)
        return jnp.concatenate([jnp.where(lo, q, zero), jnp.where(lo, zero, q)], axis=0)

    def scores(k):
        keys = rcv[TK].reshape(4 * ROWS, 128)
        return lax.dot_general(stacked_q(k), keys, NT, preferred_element_type=F32)

    def softmax_parts(s):
        m = jnp.max(s, axis=1, keepdims=True)
        p = jnp.exp2(s - m)
        return p.astype(BF16), _reciprocal(jnp.sum(p, axis=1, keepdims=True))

    def values():
        return rcv[TV].reshape(4 * ROWS, 128)

    def finish(k, o, inv_l):
        o = o * inv_l
        ctx = jnp.where(_lo_lanes(ROWS), o[:ROWS], o[ROWS:]).astype(BF16)
        if k == OWN:
            crcv[OWN] = ctx
        else:
            csnd[k - 1] = ctx
            _ctx_copy(csnd, crcv, c_send_sem, c_sems, me, k).start()

    def softmax_stage(k, slot):
        p, inv_l = softmax_parts(scores(k))
        pst[slot] = p
        lst[slot] = jnp.broadcast_to(inv_l, (2 * ROWS, 128))

    def value_stage(k, slot):
        o = jnp.dot(pst[slot], values(), preferred_element_type=F32)
        finish(k, o, lst[slot])

    _wait_bytes_of(rcv.at[TK, pl.ds(1, 3)], sems.at[SEM_K])
    softmax_stage(OWN, 0)

    gate[0].wait_send()
    send(TQ, Y)

    loads[("wo",)].wait()
    wob[0] = wo_v[pl.ds(pl.multiple_of(p0 * 128, 128), 128), :].astype(BF16)
    wob[1] = wo_v[pl.ds(pl.multiple_of((1 - p0) * 128, 128), 128), :].astype(BF16)

    _wait_bytes_of(rcv.at[TQ, D], sems.at[SEM_Q + D - 1])
    softmax_stage(D, 1)
    _wait_bytes_of(rcv.at[TV, pl.ds(1, 3)], sems.at[SEM_V])
    value_stage(D, 1)

    _wait_bytes_of(rcv.at[TQ, X], sems.at[SEM_Q + X - 1])
    _wait_bytes_of(rcv.at[TQ, Y], sems.at[SEM_Q + Y - 1])
    p, inv_l = softmax_parts(scores(X))
    o = jnp.dot(p, values(), preferred_element_type=F32)
    s_next = scores(Y)
    finish(X, o, inv_l)
    p, inv_l = softmax_parts(s_next)
    o = jnp.dot(p, values(), preferred_element_type=F32)
    finish(Y, o, inv_l)

    value_stage(OWN, 0)

    for cp in sends:
        cp.wait_send()


def _kernel_body(x_hbm, wq_hbm, wk_hbm, wv_hbm, wo_hbm, out_ref,
                 x_v, xb_v, w_v, wo_v, wob, snd, rcv, csnd, crcv, acc, pst, lst,
                 c_send_sem, c_sems):
    pl.run_scoped(
        lambda sems: _exchange_and_attend(
            x_hbm, wq_hbm, wk_hbm, wv_hbm, wo_hbm,
            x_v, xb_v, w_v, wo_v, wob, snd, rcv, csnd, crcv, pst, lst,
            c_send_sem, c_sems, sems),
        pltpu.SemaphoreType.DMA((N_SCOPED_SEMS,)))

    me = lax.axis_index("i")
    b0 = (me ^ (me >> 1)) & 1

    def out_part(k):
        return jnp.dot(crcv[k], wob[REL[k][1]], preferred_element_type=F32)

    acc[0] = out_part(OWN)
    _wait_bytes_of(crcv.at[D], c_sems.at[D - 1])
    acc[1] = out_part(D)
    _wait_bytes_of(crcv.at[X], c_sems.at[X - 1])
    out_ref[b0] = acc[0] + out_part(X)
    _wait_bytes_of(crcv.at[Y], c_sems.at[Y - 1])
    out_ref[1 - b0] = acc[1] + out_part(Y)

    for k in (D, X, Y):
        _ctx_copy(csnd, crcv, c_send_sem, c_sems, me, k).wait_send()


def pallas_dist_rope_attn_qseq_b2_sq128_d512_hq4_dh64_kernel(x, Wq, Wk, Wv, Wo):
    hbm = pl.BlockSpec(memory_space=pltpu.HBM)
    return pl.pallas_call(
        _kernel_body,
        out_shape=jax.ShapeDtypeStruct(x.shape, F32),
        in_specs=[hbm] * 5,
        out_specs=pl.BlockSpec(memory_space=pltpu.VMEM),
        scratch_shapes=[
            pltpu.VMEM((2, ROWS, DM), F32),
            pltpu.VMEM((2, ROWS, DM), BF16),
            pltpu.VMEM((3, 2, DM, 128), F32),
            pltpu.VMEM((256, DM), F32),
            pltpu.VMEM((2, 128, DM), BF16),
            pltpu.VMEM((3, 3, ROWS, 128), BF16),
            pltpu.VMEM((3, 4, ROWS, 128), BF16),
            pltpu.VMEM((3, ROWS, 128), BF16),
            pltpu.VMEM((4, ROWS, 128), BF16),
            pltpu.VMEM((2, ROWS, DM), F32),
            pltpu.VMEM((2, 2 * ROWS, 512), BF16),
            pltpu.VMEM((2, 2 * ROWS, 128), F32),
            pltpu.SemaphoreType.DMA,
            pltpu.SemaphoreType.DMA((3,)),
        ],
        compiler_params=pltpu.CompilerParams(collective_id=0),
    )(x, Wq, Wk, Wv, Wo)
```
